```python
import numpy as np

kernel_name = "dist_sparse_attn_strided_htp_bs_b2_sq256_skv256_hq4_dh64"

def setup_inputs():
    x = np.random.randn(8, 256, 512).astype(np.float32)
    Wq = np.random.randn(512, 1024).astype(np.float32) * 0.02
    K_ext = np.random.randn(8, 256, 16, 64).astype(np.float32)
    V_ext = np.random.randn(8, 256, 16, 64).astype(np.float32)
    Wo = np.random.randn(1024, 512).astype(np.float32) * 0.02
    return {"x": x, "Wq": Wq, "K_ext": K_ext, "V_ext": V_ext, "Wo": Wo}

def reference(x, Wq, K_ext, V_ext, Wo):
    B, Sq, Skv, Hq, Dh = 8, 256, 256, 16, 64
    Q = (x @ Wq).reshape(B, Sq, Hq, Dh)
    qb = (np.arange(Sq) // 64)[:, None]
    kb = (np.arange(Skv) // 64)[None, :]
    mask = (qb == kb) | ((kb % 4) == (qb % 4))
    scores = np.einsum('bihd,bjhd->bhij', Q, K_ext).astype(np.float32) * 0.125
    scores = np.where(mask[None, None, :, :], scores, -1e9)
    scores_max = scores.max(axis=-1, keepdims=True)
    w = np.exp(scores - scores_max)
    row_keep = mask.any(axis=1)
    w_sum = np.where(row_keep[None, None, :, None], w.sum(axis=-1, keepdims=True), 1.0)
    w = w / w_sum
    w = np.where(row_keep[None, None, :, None], w, 0.0)
    ctx = np.einsum('bhij,bjhd->bihd', w, V_ext).reshape(B, Sq, Hq * Dh)
    return ctx @ Wo
```

```python
import contextlib

import jax
import jax.numpy as jnp
from jax import lax
from jax.experimental import pallas as pl
from jax.experimental.pallas import tpu as pltpu

SCOPES = False
N_DEV = 4
B_LOC, SEQ, D_MODEL = 2, 256, 512
ROWS = B_LOC * SEQ
PAIR = 128
BLK = 64
HEAD_ROWS = 128
N_SLAB = D_MODEL // 128
MESH = pl.DeviceIdType.MESH
F32, BF16 = jnp.float32, jnp.bfloat16
NO_CHECKS = True
OUT_BF16 = False


def _scope(name):
    return jax.named_scope(name) if SCOPES else contextlib.nullcontext()


def _body(x_hbm, wq_hbm, kt_hbm, vt_hbm, wo_hbm, out_ref,
          x_f32, wq_f32, wo_f32, k_f32, v_f32,
          x_bf, wq_bf, wo_bf, ctx_bf, acc,
          in_sem, kv_sem, send_sem, q_sem, o_sem, entered):
    me = lax.axis_index("i")
    left = (me + N_DEV - 1) % N_DEV
    right = (me + 1) % N_DEV
    diag = (me + 2) % N_DEV
    nbr = (right, left)

    head, rest = pl.ds(0, HEAD_ROWS), pl.ds(HEAD_ROWS, D_MODEL - HEAD_ROWS)
    ld_wq0 = pltpu.make_async_copy(wq_hbm.at[head], wq_f32.at[head], in_sem.at[0])
    ld_wq1 = pltpu.make_async_copy(wq_hbm.at[rest], wq_f32.at[rest], in_sem.at[1])
    ld_wo = pltpu.make_async_copy(wo_hbm, wo_f32, in_sem.at[2])
    ld_x = pltpu.make_async_copy(x_hbm, x_f32, in_sem.at[3])
    ld_wq0.start()
    ld_wq1.start()

    stage_pairs = (((me, 0), (me, 1)), ((left, 0), (right, 1)),
                   ((left, 1), (right, 0)), ((diag, 0), (diag, 1)))

    def kv_copies(s):
        cps = []
        for j, (chip, half) in enumerate(stage_pairs[s]):
            rows = pl.ds(pl.multiple_of((2 * chip + half) * PAIR, PAIR), PAIR)
            for src, dst in ((kt_hbm, k_f32), (vt_hbm, v_f32)):
                cps.append(pltpu.make_async_copy(
                    src.at[pl.ds(B_LOC * me, B_LOC), rows], dst.at[s, j], kv_sem.at[s]))
        return cps

    def rdma(d, src, dst, sem):
        return pltpu.make_async_remote_copy(src, dst, send_sem.at[d], sem,
                                            device_id=(nbr[d],), device_id_type=MESH)

    def q_first(d, rows):
        return rdma(d, wq_bf.at[0, d, rows], wq_bf.at[1, d, rows], q_sem.at[0])

    def q_second(d):
        return rdma(d, wq_bf.at[0, 1 - d], wq_bf.at[2, d], q_sem.at[1])

    def q_fwd(d):
        return rdma(d, wq_bf.at[1, d], wq_bf.at[3, d], q_sem.at[2])

    def o_first(d):
        return rdma(d, wo_bf.at[0, :, d], wo_bf.at[1, :, d], o_sem.at[0])

    def o_second(d):
        return rdma(d, wo_bf.at[0, :, 1 - d], wo_bf.at[2, :, d], o_sem.at[1])

    def o_fwd(d, n):
        return rdma(d, wo_bf.at[1, n, d], wo_bf.at[3, n, d], o_sem.at[2 + n])

    def wait_landed(buf, sem):
        pltpu.make_async_copy(buf, buf, sem).wait()

    bar = pltpu.get_barrier_semaphore()

    def signal(sem, dev):
        pl.semaphore_signal(sem, inc=1, device_id=(dev,), device_id_type=MESH)

    @pl.when(me == 0)
    def _():
        signal(bar, 1)
        signal(bar, 3)

    @pl.when(me % 2 == 1)
    def _():
        signal(bar, 2)
        pl.semaphore_wait(bar, 1)
        signal(entered, 0)

    @pl.when(me == 2)
    def _():
        pl.semaphore_wait(bar, 2)
        signal(entered, 1)
        signal(entered, 3)

    def cast_wq(rows):
        for h in range(2):
            wq_bf[0, h, rows, :] = wq_f32[rows, h * PAIR:(h + 1) * PAIR].astype(BF16)

    with _scope("ld_wq0"):
        ld_wq0.wait()
    cast_wq(head)

    @pl.when(me != 0)
    def _():
        @pl.when(me != 1)
        def _():
            q_first(0, head).start()

        @pl.when(me != 3)
        def _():
            q_first(1, head).start()

    ld_wo.start()
    ld_x.start()
    with _scope("ld_wq1"):
        ld_wq1.wait()
    cast_wq(rest)
    for cp in kv_copies(0):
        cp.start()

    def send_q(d, with_head):
        if with_head:
            q_first(d, head).start()
        q_first(d, rest).start()
        q_second(d).start()

    with _scope("handshake"):
        @pl.when(me == 0)
        def _():
            pl.semaphore_wait(entered, 2)
            send_q(0, True)
            send_q(1, True)

        @pl.when(me == 1)
        def _():
            send_q(1, False)
            pl.semaphore_wait(entered, 1)
            send_q(0, True)

        @pl.when(me == 2)
        def _():
            send_q(0, False)
            send_q(1, False)

        @pl.when(me == 3)
        def _():
            send_q(0, False)
            pl.semaphore_wait(entered, 1)
            send_q(1, True)

    for s in range(1, 4):
        for cp in kv_copies(s):
            cp.start()

    with _scope("ld_wo"):
        ld_wo.wait()
    for n in range(N_SLAB):
        for h in range(2):
            wo_bf[0, n, h] = wo_f32[h * PAIR:(h + 1) * PAIR, n * 128:(n + 1) * 128].astype(BF16)
    o_first(0).start()
    o_first(1).start()

    with _scope("ld_x"):
        ld_x.wait()
    x_bf[...] = (x_f32[...] * 0.125).astype(BF16)

    lane = lax.broadcasted_iota(jnp.int32, (BLK, 128), 1)
    lo = lane < BLK
    lane2 = lax.broadcasted_iota(jnp.int32, (128, 128), 1)
    lo2 = lane2 < BLK

    row2 = lax.broadcasted_iota(jnp.int32, (128, 128), 0) < BLK
    on_diag = row2 == lo2
    tiles = [(j, b, t) for j in range(2) for b in range(B_LOC) for t in range(SEQ // 128)]

    def attention(s):
        w = jnp.concatenate([wq_bf[s, 0], wq_bf[s, 1]], axis=1)
        q = jnp.dot(x_bf[...], w, preferred_element_type=F32)
        for cp in kv_copies(s):
            cp.wait()
        scores = []
        for j, b, t in tiles:
            r0 = b * SEQ + t * 128
            qt = q[r0:r0 + 128, j * PAIR:(j + 1) * PAIR]
            k = k_f32[s, j, b, :, t * 128:(t + 1) * 128].T
            for keys, qm in ((jnp.where(lo, k[:BLK], k[BLK:]), jnp.where(on_diag, qt, 0.0)),
                             (jnp.where(lo, k[BLK:], k[:BLK]), jnp.where(on_diag, 0.0, qt))):
                scores.append(lax.dot_general(keys.astype(BF16), qm.astype(BF16),
                                              (((1,), (1,)), ((), ())), preferred_element_type=F32))
        probs = []
        for sc in scores:
            p = jnp.exp(sc - jnp.max(sc, axis=0, keepdims=True))
            inv = 1.0 / jnp.sum(p, axis=0, keepdims=True)
            pd = jnp.concatenate([jnp.where(lo, p, 0.0), jnp.where(lo, 0.0, p)], axis=0)
            probs.append((pd.astype(BF16), inv))
        outs = []
        for i, (j, b, t) in enumerate(tiles):
            v = v_f32[s, j, b, :, t * 128:(t + 1) * 128]
            (pd, inv_d), (pa, inv_a) = probs[2 * i], probs[2 * i + 1]
            cd = jnp.dot(jnp.where(lo, v[:BLK], v[BLK:]).astype(BF16), pd, preferred_element_type=F32) * inv_d
            ca = jnp.dot(jnp.where(lo, v[BLK:], v[:BLK]).astype(BF16), pa, preferred_element_type=F32) * inv_a
            outs.append(jnp.concatenate([jnp.where(lo, cd, ca), jnp.where(lo, ca, cd)], axis=0))
        for ct, (j, b, t) in zip(outs, tiles):
            r0 = b * SEQ + t * 128
            ctx_bf[s, r0:r0 + 128, j * PAIR:(j + 1) * PAIR] = ct.T.astype(BF16)

    def out_proj(s, n):
        w = wo_bf[s, n].reshape(2 * PAIR, 128)
        return jnp.dot(ctx_bf[s], w, preferred_element_type=F32)

    def slab(n):
        return slice(n * 128, (n + 1) * 128)

    with _scope("att0"):
        attention(0)
    with _scope("w_q0"):
        wait_landed(wq_bf.at[1], q_sem.at[0])
    for d in range(2):
        q_fwd(d).start()
        o_second(d).start()
    with _scope("att1"):
        attention(1)
        for n in range(N_SLAB):
            acc[:, slab(n)] = out_proj(0, n)
    with _scope("w_q1"):
        wait_landed(wq_bf.at[2], q_sem.at[1])
    with _scope("att2"):
        attention(2)
    with _scope("w_o0"):
        wait_landed(wo_bf.at[1], o_sem.at[0])
    for n in range(N_SLAB):
        for d in range(2):
            o_fwd(d, n).start()
    with _scope("op1"):
        for n in range(N_SLAB):
            acc[:, slab(n)] += out_proj(1, n)
    with _scope("w_q2"):
        wait_landed(wq_bf.at[3], q_sem.at[2])
    with _scope("att3"):
        attention(3)
    with _scope("w_o1"):
        wait_landed(wo_bf.at[2], o_sem.at[1])
    with _scope("op2"):
        for n in range(N_SLAB):
            acc[:, slab(n)] += out_proj(2, n)
    for n in range(N_SLAB):
        with _scope(f"w_f{n}"):
            wait_landed(wo_bf.at[3, n], o_sem.at[2 + n])
        w = wo_bf[3, n].reshape(2 * PAIR, 128)
        for r in range(2):
            rows = slice(r * SEQ, (r + 1) * SEQ)
            out_ref[r, :, slab(n)] = (acc[rows, slab(n)] + jnp.dot(
                ctx_bf[3, rows], w, preferred_element_type=F32)).astype(out_ref.dtype)
    with _scope("w_send"):
        for d in range(2):
            q_first(d, head).wait_send()
            q_first(d, rest).wait_send()
            q_second(d).wait_send()
            q_fwd(d).wait_send()
            o_first(d).wait_send()
            o_second(d).wait_send()
            for n in range(N_SLAB):
                o_fwd(d, n).wait_send()


def pallas_dist_sparse_attn_strided_htp_bs_b2_sq256_skv256_hq4_dh64_kernel(x, Wq, K_ext, V_ext, Wo):
    n_b, _, n_h, d_h = K_ext.shape
    kt = jnp.transpose(K_ext, (0, 2, 3, 1)).reshape(n_b, n_h * d_h, SEQ)
    vt = jnp.transpose(V_ext, (0, 2, 3, 1)).reshape(n_b, n_h * d_h, SEQ)
    hbm = pl.BlockSpec(memory_space=pltpu.HBM)
    return pl.pallas_call(
        _body,
        out_shape=jax.ShapeDtypeStruct((B_LOC, SEQ, D_MODEL), BF16 if OUT_BF16 else F32),
        in_specs=[hbm] * 5,
        out_specs=pl.BlockSpec(memory_space=pltpu.VMEM),
        scratch_shapes=[
            pltpu.VMEM((ROWS, D_MODEL), F32),
            pltpu.VMEM((D_MODEL, 2 * PAIR), F32),
            pltpu.VMEM((2 * PAIR, D_MODEL), F32),
            pltpu.VMEM((4, 2, B_LOC, PAIR, SEQ), F32),
            pltpu.VMEM((4, 2, B_LOC, PAIR, SEQ), F32),
            pltpu.VMEM((ROWS, D_MODEL), BF16),
            pltpu.VMEM((4, 2, D_MODEL, PAIR), BF16),
            pltpu.VMEM((4, N_SLAB, 2, PAIR, 128), BF16),
            pltpu.VMEM((4, ROWS, 2 * PAIR), BF16),
            pltpu.VMEM((ROWS, D_MODEL), F32),
            pltpu.SemaphoreType.DMA((4,)),
            pltpu.SemaphoreType.DMA((4,)),
            pltpu.SemaphoreType.DMA((2,)),
            pltpu.SemaphoreType.DMA((3,)),
            pltpu.SemaphoreType.DMA((2 + N_SLAB,)),
            pltpu.SemaphoreType.REGULAR,
        ],
        compiler_params=pltpu.CompilerParams(
            collective_id=0, vmem_limit_bytes=48 * 1024 * 1024,
            disable_bounds_checks=NO_CHECKS, disable_semaphore_checks=NO_CHECKS),
    )(x.reshape(ROWS, D_MODEL), Wq, kt, vt, Wo)
```

```python
import contextlib

import jax
import jax.numpy as jnp
from jax import lax
from jax.experimental import pallas as pl
from jax.experimental.pallas import tpu as pltpu

SCOPES = False
NO_CHECKS = True
OUT_BF16 = True
FORCE_SPILL = False

N_DEV = 4
B_LOC, SEQ, D_MODEL = 2, 256, 512
ROWS = B_LOC * SEQ
BLK = 64
T = 128
N_T = D_MODEL // T
N_G = 2 * N_T
MESH = pl.DeviceIdType.MESH
F32, BF16, I32 = jnp.float32, jnp.bfloat16, jnp.int32

HI = 0x78007800
KEEP = 0x87FF87FF - (1 << 32)
SPILLED = 0xFF
srl = lax.shift_right_logical


def _scope(name):
    return jax.named_scope(name) if SCOPES else contextlib.nullcontext()


def _vregs(a):
    return [a[i:i + 8] for i in range(0, a.shape[0], 8)]


def _both_halves(base):
    return (base << 7) | (base << 23)


def _base(rows, margin):
    top = jnp.max(jnp.abs(rows), axis=0, keepdims=True)
    return jnp.maximum((srl(pltpu.bitcast(top, I32), 23) & 0xFF) + (margin - 15), 0)


def _pack_group(rows, base, g):
    words = pltpu.bitcast(rows.astype(BF16), I32)
    both = jnp.broadcast_to(_both_halves(base), (8, T))
    sub = lax.broadcasted_iota(I32, (8, T), 0)
    low, notes = [], []
    for i, w in enumerate(_vregs(words)):
        t = w - both
        d = t & HI
        low.append(t & KEEP)
        notes.append(jnp.where(d != 0, d | (sub + (32 * g + 8 * i)), 0))
    a, b, c, e = low
    payload = [a | ((e << 11) & HI), b | ((e << 7) & HI),
               c | ((e << 3) & 0x38003800) | (srl(e, 1) & 0x40004000)]
    return words, jnp.concatenate(payload, axis=0), notes


def _meta(base, notes):
    best, total, count = notes[0], notes[0], jnp.minimum(notes[0], 1)
    for c in notes[1:]:
        best, total, count = jnp.maximum(best, c), total + c, count + jnp.minimum(c, 1)
    first = jnp.max(best, axis=0, keepdims=True)
    second = jnp.sum(total, axis=0, keepdims=True) - first
    over = jnp.sum(count, axis=0, keepdims=True) > 2
    meta = base
    for k, s in enumerate((first, second)):
        n_lo, n_hi = srl(s, 11) & 15, srl(s, 27) & 15
        n = n_lo | n_hi
        over = over | ((n_lo != 0) & (n_hi != 0)) | ((n > 1) & (n < 10))
        code = (s & 255) | ((n & 7) << 8) | jnp.where(n_hi != 0, 1 << 11, 0)
        meta = meta | (code << (8 + 12 * k))
    return meta, over


def _spill_group(words, base):
    both = jnp.broadcast_to(_both_halves(base), (8, T))
    a, b, c, e = [(w - both) & HI for w in _vregs(words)]
    return srl(a, 11) | srl(b, 7) | srl(c, 3) | (e << 1)


def _offsets(meta):
    m = jnp.broadcast_to(meta, (8, T))
    both = _both_halves(m & 0xFF)
    sub = lax.broadcasted_iota(I32, (8, T), 0)
    keys, adds = [], []
    for k in range(2):
        code = srl(m, 8 + 12 * k)
        n = srl(code, 8) & 7
        keys.append((code & 255) - sub)
        adds.append(both + (jnp.where(n > 1, n + 8, n) << (11 + (srl(code, 7) & 16))))
    return [jnp.concatenate(
        [jnp.where(keys[0] == i, adds[0], jnp.where(keys[1] == i, adds[1], both))
         for i in range(32 * g, 32 * g + 32, 8)], axis=0) for g in range(N_G)]


def _spilled_bits(x):
    return jnp.concatenate([d & HI for d in (x << 11, x << 7, x << 3, srl(x, 1))], axis=0)


def _unpack_group(payload, offsets):
    a, b, c = _vregs(payload)
    e = (srl(a, 11) & 0x000F000F) | (srl(b, 7) & 0x00F000F0) | (srl(c, 3) & 0x0F000F00)
    return (jnp.concatenate([a, b, c, e + HI], axis=0) & KEEP) + offsets


def _body(x_hbm, wq_hbm, kt_hbm, vt_hbm, wo_hbm, out_ref,
          x_f32, wq_f32, wo_f32, k_f32, v_f32, x_w, ctx_w, acc,
          own_w, offs, pay, meta, spill,
          in_sem, kv_sem, send_sem, spill_send_sem, pay_sem, last_sem, meta_sem, spill_sem, entered):
    me = lax.axis_index("i")
    left = (me + N_DEV - 1) % N_DEV
    right = (me + 1) % N_DEV
    diag = (me + 2) % N_DEV
    WQ, WO = 0, 1
    u = (me == 1).astype(I32)

    def ld_wq(half, rows, sem):
        cols = pl.ds(pl.multiple_of(half * T, T), T)
        return pltpu.make_async_copy(wq_hbm.at[rows, cols], wq_f32.at[half, rows], in_sem.at[sem])

    chunks = ((u, 0, 1), (u, 1, 3), (1 - u, 0, 3), (u, 3, N_G), (1 - u, 3, N_G))
    wq_loads = [ld_wq(half, pl.ds(g0 * BLK, (g1 - g0) * BLK), i)
                for i, (half, g0, g1) in enumerate(chunks)]
    ld_wo = pltpu.make_async_copy(wo_hbm, wo_f32, in_sem.at[5])
    ld_x = pltpu.make_async_copy(x_hbm, x_f32, in_sem.at[6])
    for cp in wq_loads:
        cp.start()

    stage_pairs = (((me, 0), (me, 1)), ((left, 0), (right, 1)),
                   ((left, 1), (right, 0)), ((diag, 0), (diag, 1)))

    def kv_copies(s):
        cps = []
        for j, (chip, half) in enumerate(stage_pairs[s]):
            rows = pl.ds(pl.multiple_of((2 * chip + half) * T, T), T)
            for src, dst in ((kt_hbm, k_f32), (vt_hbm, v_f32)):
                cps.append(pltpu.make_async_copy(
                    src.at[pl.ds(B_LOC * me, B_LOC), rows], dst.at[s, j], kv_sem.at[s]))
        return cps

    def route(w, s, d):
        src = {1: (0, d), 2: (0, 1 - d), 3: (1, d)}[s]
        return (w,) + src, (w, s, d), (jnp.where(d == 0, right, left),)

    def send_pay(w, s, d, groups=pl.ds(0, N_G), sem=None):
        (sw, ss, sj), (dw, ds, dj), dev = route(w, s, d)
        return pltpu.make_async_remote_copy(
            pay.at[sw, ss, groups, sj], pay.at[dw, ds, groups, dj], send_sem,
            pay_sem.at[3 * w + s - 1] if sem is None else sem, device_id=dev, device_id_type=MESH)

    def send_meta(w, s, d):
        src, dst, dev = route(w, s, d)
        return pltpu.make_async_remote_copy(
            meta.at[src], meta.at[dst], send_sem, meta_sem.at[3 * w + s - 1],
            device_id=dev, device_id_type=MESH)

    def send_spill(w, s, d):
        src, dst, dev = route(w, s, d)
        return pltpu.make_async_remote_copy(
            spill.at[src], spill.at[dst], spill_send_sem, spill_sem.at[6 * w + 2 * (s - 1) + d],
            device_id=dev, device_id_type=MESH)

    def start_side(w, s, d, spilled):
        send_meta(w, s, d).start()

        @pl.when(spilled)
        def _():
            send_spill(w, s, d).start()

    def wait_landed(buf, sem):
        pltpu.make_async_copy(buf, buf, sem).wait()

    def pack_group(w, half, g, rows, base):
        words, payload, notes = _pack_group(rows, base, g)
        own_w[w, half, g] = words
        pay[w, 0, g, half] = payload
        return notes

    def seal(w, half, base, notes):
        m, over = _meta(base, notes)
        spilled = jnp.max(over.astype(F32)) > (-1 if FORCE_SPILL else 0)
        meta[w, 0, half] = jnp.where(spilled, base | (SPILLED << 8), m)

        @pl.when(spilled)
        def _():
            for g in range(N_G):
                spill[w, 0, half, g] = _spill_group(own_w[w, half, g], base)
        return spilled

    def receive_side(w, s):
        wait_landed(meta.at[w, s], meta_sem.at[3 * w + s - 1])
        flags = []
        for d in range(2):
            for g, o in enumerate(_offsets(meta[w, s, d])):
                offs[d, g] = o
            flags.append(srl(meta[w, s, d, 0, 0], 8) == SPILLED)
        for d in range(2):
            @pl.when(flags[d])
            def _():
                send_spill(w, s, d).wait_recv()
                for g in range(N_G):
                    offs[d, g] += _spilled_bits(spill[w, s, d, g])
        return flags

    def weights(w, s, d, g):
        words = own_w[w, d, g] if s == 0 else _unpack_group(pay[w, s, g, d], offs[d, g])
        return pltpu.bitcast(words, BF16)

    bar = pltpu.get_barrier_semaphore()

    def signal(sem, dev):
        pl.semaphore_signal(sem, inc=1, device_id=(dev,), device_id_type=MESH)

    @pl.when(me == 0)
    def _():
        signal(bar, 1)
        signal(bar, 3)

    @pl.when(me % 2 == 1)
    def _():
        signal(bar, 2)
        pl.semaphore_wait(bar, 1)
        signal(entered, 0)

    @pl.when(me == 2)
    def _():
        pl.semaphore_wait(bar, 2)
        signal(entered, 1)
        signal(entered, 3)

    def send_chunk(i):
        half, g0, g1 = chunks[i]
        return send_pay(WQ, 1, half, pl.ds(g0, g1 - g0))

    early = (me != 0, me != 0, me == 2, me != 0, me == 2)
    bases, notes = [None, None], [[], []]
    for i, (half, g0, g1) in enumerate(chunks):
        k = (0, 0, 1, 0, 1)[i]
        with _scope(f"ld_{i}"):
            wq_loads[i].wait()
        if g0 == 0:
            bases[k] = _base(wq_f32[half, :g1 * BLK], 1)
        for g in range(g0, g1):
            notes[k] += pack_group(WQ, half, g, wq_f32[half, g * BLK:(g + 1) * BLK], bases[k])

        @pl.when(early[i])
        def _():
            send_chunk(i).start()

        if i == 2:
            ld_wo.start()
        if i == 4:
            ld_x.start()

    with _scope("handshake"):
        @pl.when(me == 0)
        def _():
            pl.semaphore_wait(entered, 2)
            for i in range(len(chunks)):
                send_chunk(i).start()

        @pl.when(me % 2 == 1)
        def _():
            pl.semaphore_wait(entered, 1)
            send_chunk(2).start()
            send_chunk(4).start()

    q_spilled_u = seal(WQ, u, bases[0], notes[0])
    q_spilled_v = seal(WQ, 1 - u, bases[1], notes[1])
    start_side(WQ, 1, u, q_spilled_u)
    start_side(WQ, 1, 1 - u, q_spilled_v)
    start_side(WQ, 2, u, q_spilled_v)
    start_side(WQ, 2, 1 - u, q_spilled_u)
    for d in range(2):
        send_pay(WQ, 2, d).start()

    with _scope("ld_wo"):
        ld_wo.wait()
    for cp in kv_copies(0):
        cp.start()
    o_spilled = []
    for half in range(2):
        groups = [wo_f32[half * T + g % 2 * BLK:half * T + (g % 2 + 1) * BLK, g // 2 * T:(g // 2 + 1) * T]
                  for g in range(N_G)]
        base = _base(jnp.concatenate(groups, axis=0), 0)
        o_spilled.append(seal(WO, half, base, [
            n for g in range(N_G) for n in pack_group(WO, half, g, groups[g], base)]))
        start_side(WO, 1, half, o_spilled[half])
        send_pay(WO, 1, half).start()

    with _scope("ld_x"):
        ld_x.wait()
    for cp in kv_copies(1):
        cp.start()
    x_w[...] = pltpu.bitcast((x_f32[...] * 0.125).astype(BF16), I32)

    lo = lax.broadcasted_iota(I32, (BLK, T), 1) < BLK
    on_diag = ((lax.broadcasted_iota(I32, (T, T), 0) < BLK)
               == (lax.broadcasted_iota(I32, (T, T), 1) < BLK))
    tiles = [(j, b, t) for j in range(2) for b in range(B_LOC) for t in range(SEQ // T)]

    def attention(s):
        w = jnp.concatenate(
            [jnp.concatenate([weights(WQ, s, d, g) for g in range(N_G)], axis=0) for d in range(2)],
            axis=1)
        q = jnp.dot(pltpu.bitcast(x_w[...], BF16), w, preferred_element_type=F32)
        for cp in kv_copies(s):
            cp.wait()
        if s + 2 < 4:
            for cp in kv_copies(s + 2):
                cp.start()
        scores = []
        for j, b, t in tiles:
            r0 = b * SEQ + t * T
            qt = q[r0:r0 + T, j * T:(j + 1) * T]
            k = k_f32[s, j, b, :, t * T:(t + 1) * T].T
            for keys, qm in ((jnp.where(lo, k[:BLK], k[BLK:]), jnp.where(on_diag, qt, 0.0)),
                             (jnp.where(lo, k[BLK:], k[:BLK]), jnp.where(on_diag, 0.0, qt))):
                scores.append(lax.dot_general(keys.astype(BF16), qm.astype(BF16),
                                              (((1,), (1,)), ((), ())), preferred_element_type=F32))
        probs = []
        for sc in scores:
            p = jnp.exp(sc - jnp.max(sc, axis=0, keepdims=True))
            inv = 1.0 / jnp.sum(p, axis=0, keepdims=True)
            pd = jnp.concatenate([jnp.where(lo, p, 0.0), jnp.where(lo, 0.0, p)], axis=0)
            probs.append((pd.astype(BF16), inv))
        outs = []
        for i, (j, b, t) in enumerate(tiles):
            v = v_f32[s, j, b, :, t * T:(t + 1) * T]
            (pd, inv_d), (pa, inv_a) = probs[2 * i], probs[2 * i + 1]
            cd = jnp.dot(jnp.where(lo, v[:BLK], v[BLK:]).astype(BF16), pd,
                         preferred_element_type=F32) * inv_d
            ca = jnp.dot(jnp.where(lo, v[BLK:], v[:BLK]).astype(BF16), pa,
                         preferred_element_type=F32) * inv_a
            outs.append((jnp.where(lo, cd, ca), jnp.where(lo, ca, cd)))
        n = len(tiles) // 2
        for i, (_, b, t) in enumerate(tiles[:n]):
            r0 = (b * SEQ + t * T) // 2
            for h in range(2):
                ct = jnp.concatenate([outs[i][h], outs[n + i][h]], axis=0)
                ctx_w[s, r0:r0 + T // 2, h * T:(h + 1) * T] = pltpu.bitcast(ct.T.astype(BF16), I32)

    def wo_tile(s, g):
        return jnp.concatenate([weights(WO, s, d, g) for d in range(2)], axis=0)

    def out_proj(s):
        w = jnp.concatenate(
            [jnp.concatenate([wo_tile(s, 2 * t), wo_tile(s, 2 * t + 1)], axis=0) for t in range(N_T)],
            axis=1)
        return jnp.dot(pltpu.bitcast(ctx_w[s], BF16), w, preferred_element_type=F32)

    def wait_pay(w, s):
        wait_landed(pay.at[w, s], pay_sem.at[3 * w + s - 1])

    last = ((0, 2), (2, 4), (4, 6), (6, 7), (7, 8))

    def last_copy(d, i):
        g0, g1 = last[i]
        return send_pay(WO, 3, d, pl.ds(g0, g1 - g0), last_sem.at[i])

    with _scope("att0"):
        attention(0)
    with _scope("w_q1"):
        q_fwd_spilled = receive_side(WQ, 1)
        wait_pay(WQ, 1)
    for d in range(2):
        start_side(WQ, 3, d, q_fwd_spilled[d])
        send_pay(WQ, 3, d).start()
        start_side(WO, 2, d, o_spilled[1 - d])
        send_pay(WO, 2, d).start()
    with _scope("att1"):
        attention(1)
    with _scope("w_q2"):
        receive_side(WQ, 2)
        wait_pay(WQ, 2)
    with _scope("att2"):
        attention(2)
    with _scope("w_o1"):
        o_fwd_spilled = receive_side(WO, 1)
        wait_pay(WO, 1)
    for d in range(2):
        start_side(WO, 3, d, o_fwd_spilled[d])
    for i in range(len(last)):
        for d in range(2):
            last_copy(d, i).start()
    with _scope("op01"):
        acc[...] = out_proj(0) + out_proj(1)
    with _scope("w_q3"):
        receive_side(WQ, 3)
        wait_pay(WQ, 3)
    with _scope("att3"):
        attention(3)
    with _scope("w_o2"):
        receive_side(WO, 2)
        wait_pay(WO, 2)
    with _scope("op2"):
        acc[...] += out_proj(2)
    receive_side(WO, 3)
    for spilled in [q_spilled_u, q_spilled_v] * 2 + o_spilled * 2 + q_fwd_spilled + o_fwd_spilled:
        @pl.when(spilled)
        def _():
            send_spill(WQ, 1, 0).wait_send()
    for i, (g0, g1) in enumerate(last):
        with _scope(f"w_f{i}"):
            wait_landed(pay.at[WO, 3, pl.ds(g0, g1 - g0)], last_sem.at[i])
        w = jnp.concatenate([wo_tile(3, g) for g in range(g0, g1)], axis=0)
        cols = slice(g0 // 2 * T, (g0 // 2 + 1) * T)
        step = T * (g1 - g0)
        for r in range(0, ROWS, step):
            c = ctx_w[3, r // 2:(r + step) // 2, g0 % 2 * T:g0 % 2 * T + step]
            y = acc[r:r + step, cols] + jnp.dot(pltpu.bitcast(c, BF16), w, preferred_element_type=F32)
            if g1 % 2:
                acc[r:r + step, cols] = y
            else:
                out_ref[r // SEQ, r % SEQ:r % SEQ + step, cols] = y.astype(out_ref.dtype)
    with _scope("w_send"):
        for i in range(len(chunks)):
            send_chunk(i).wait_send()
        for d in range(2):
            for w, s in ((WQ, 2), (WQ, 3), (WO, 1), (WO, 2)):
                send_pay(w, s, d).wait_send()
            for i in range(len(last)):
                last_copy(d, i).wait_send()
            for w in range(2):
                for s in range(1, 4):
                    send_meta(w, s, d).wait_send()


def pallas_dist_sparse_attn_strided_htp_bs_b2_sq256_skv256_hq4_dh64_kernel(x, Wq, K_ext, V_ext, Wo):
    n_b, _, n_h, d_h = K_ext.shape
    kt = jnp.transpose(K_ext, (0, 2, 3, 1)).reshape(n_b, n_h * d_h, SEQ)
    vt = jnp.transpose(V_ext, (0, 2, 3, 1)).reshape(n_b, n_h * d_h, SEQ)
    dma = pltpu.SemaphoreType.DMA
    return pl.pallas_call(
        _body,
        out_shape=jax.ShapeDtypeStruct((B_LOC, SEQ, D_MODEL), BF16 if OUT_BF16 else F32),
        in_specs=[pl.BlockSpec(memory_space=pltpu.HBM)] * 5,
        out_specs=pl.BlockSpec(memory_space=pltpu.VMEM),
        scratch_shapes=[
            pltpu.VMEM((ROWS, D_MODEL), F32),
            pltpu.VMEM((2, D_MODEL, T), F32),
            pltpu.VMEM((2 * T, D_MODEL), F32),
            pltpu.VMEM((4, 2, B_LOC, T, SEQ), F32),
            pltpu.VMEM((4, 2, B_LOC, T, SEQ), F32),
            pltpu.VMEM((ROWS // 2, D_MODEL), I32),
            pltpu.VMEM((4, ROWS // 2, 2 * T), I32),
            pltpu.VMEM((ROWS, D_MODEL), F32),
            pltpu.VMEM((2, 2, N_G, 32, T), I32),
            pltpu.VMEM((2, N_G, 32, T), I32),
            pltpu.VMEM((2, 4, N_G, 2, 24, T), I32),
            pltpu.VMEM((2, 4, 2, 1, T), I32),
            pltpu.VMEM((2, 4, 2, N_G, 8, T), I32) ,
            dma((7,)), dma((4,)), dma, dma, dma((5,)), dma((5,)), dma((6,)), dma((12,)),
            pltpu.SemaphoreType.REGULAR,
        ],
        compiler_params=pltpu.CompilerParams(
            collective_id=0, vmem_limit_bytes=48 * 1024 * 1024,
            disable_bounds_checks=NO_CHECKS, disable_semaphore_checks=NO_CHECKS),
    )(x.reshape(ROWS, D_MODEL), Wq, kt, vt, Wo)
```

```python
import jax
import jax.numpy as jnp
from jax import lax
from jax.experimental import pallas as pl
from jax.experimental.pallas import tpu as pltpu

N_DEV = 4
B_LOC, SEQ, D_MODEL = 2, 256, 512
ROWS = B_LOC * SEQ
BLK = 64
T = 128
N_G = 8
WQ, WO = 0, 1
F32, BF16, I32 = jnp.float32, jnp.bfloat16, jnp.int32

CHUNKS = ((0, 0, 1), (0, 1, 3), (0, 3, 8), (1, 0, 5), (0, 8, 16), (1, 5, 16))
AHEAD = 5
LAST = ((2, 0, 4), (2, 4, 8), (3, 0, 2), (3, 2, 4), (3, 4, 6), (3, 6, 8))

LOW = 0x00FF00FF
SIGN = 0x80008000 - (1 << 32)
ONES = 0x11111111
CODE_ROWS = 48
MAX_BITS = 128 + 21
RAW = 0xFF
srl = lax.shift_right_logical


def _regs(a):
    return [a[i:i + 8] for i in range(0, a.shape[0], 8)]


def _shift(a, n):
    return a if n == 0 else a << n if n > 0 else srl(a, -n)


def _low_bytes(words):
    v = _regs(words)
    return jnp.concatenate([(a & LOW) | ((b & LOW) << 8) for a, b in zip(v[::2], v[1::2])], axis=0)


def _high_bytes(words):
    v = _regs(words)
    return jnp.concatenate([(srl(a, 8) & LOW) | (b & ~LOW) for a, b in zip(v[::2], v[1::2])], axis=0)


def _pivot(rows):
    top = jnp.sum(jnp.abs(rows), axis=0, keepdims=True) * (11.0 / rows.shape[0])
    return srl(pltpu.bitcast(top, I32), 16) & 0x7FFF


def _encode(piece, top):
    words = _regs(piece)
    tops = jnp.broadcast_to(top | (top << 16), (8, T))
    one = jnp.ones((8, T), I32)
    signs, stream, total, wide, longest = [0, 0], [], 0, 0, 0
    for g in reversed(range(N_G)):
        steps = 0
        for i in range(4):
            w = words[4 * g + i]
            signs[g // 4] = signs[g // 4] | _shift(w & SIGN, -((4 * g + i) % 16))
            below = tops - (w & ~SIGN)
            wide = wide | below | (below + 0x01000100)
            steps = steps | _shift(below & 0x0F000F00, 4 * i - 8)
        ge4 = (srl(steps, 2) | srl(steps, 3)) & ONES
        is0 = (((steps | srl(steps, 1)) & ONES) | ge4) ^ ONES
        lengths = steps + ge4 + (is0 << 2)
        for run in (lengths, srl(lengths, 16)):
            bits, code = 0, 0
            for e in (12, 8, 4, 0):
                bits = bits + (_shift(run, -e) & 15)
                code = code | (one << (bits & 31))
            total, longest = total + bits, longest | bits
            carry = [srl(code, 1)] + [srl(s, -bits & 31) for s in stream]
            stream = [c | (s << (bits & 31)) for c, s in zip(carry, stream)] + carry[len(stream):5]
    note = jnp.where(stream[4] != 0, (stream[4] << 3) | lax.broadcasted_iota(I32, (8, T), 0), 0)
    first = jnp.max(note, axis=0, keepdims=True)
    second = jnp.sum(note, axis=0, keepdims=True) - first
    crowded = jnp.sum(jnp.minimum(note, 1), axis=0, keepdims=True) > 2
    misfit = ((srl(wide, 12) & 0x000F000F) != 0) | (longest > 31) | (total > MAX_BITS) | crowded
    meta = jnp.concatenate([(first << 8) | (top & 0xFF), (second << 8) | srl(top, 8)], axis=0)
    return jnp.concatenate(signs + stream[:4], axis=0), meta, misfit


def _decode(codes, metas):
    s0, s1, *stream = [jnp.concatenate(v, axis=0) for v in zip(*map(_regs, codes))]
    m0, m1 = (jnp.concatenate([jnp.broadcast_to(m[i:i + 1], (8, T)) for m in metas], axis=0)
              for i in range(2))
    sub = lax.broadcasted_iota(I32, m0.shape, 0) & 7
    stream.append(jnp.where((srl(m0, 8) & 7) == sub, srl(m0, 11), 0)
                  | jnp.where((srl(m1, 8) & 7) == sub, srl(m1, 11), 0))
    top = (m0 & 0xFF) | ((m1 & 0x7F) << 8)
    tops = top | (top << 16)
    words, at = [], None
    for g in range(N_G):
        runs = []
        for to_come in (2 * (N_G - g) - 1, 2 * (N_G - g) - 2):
            r = stream[0] if at is None else srl(stream[0], at) | ((stream[1] << 1) << (31 - at))
            ends = []
            for e in (12, 8, 4, 0):
                rest = r & (r - 1)
                ends.append(srl(pltpu.bitcast((r ^ rest).astype(F32), I32), 23 - e))
                r = rest
            head = ends[0] + ends[1] + ends[2]
            runs.append(head + ends[3] - srl(head, 4) - (126 << 12))
            if to_come:
                at = ends[3] - 126 if at is None else at + ends[3] - 126
                stream = [jnp.where(at > 31, b, a)
                          for a, b in zip(stream, stream[1:])][:to_come + 1] + stream[4:]
                at = at & 31
        lengths = (runs[0] << 16) + runs[1]
        b2, b3 = srl(lengths, 2), srl(lengths, 3)
        is4 = b2 & ~(b3 | srl(lengths, 1) | lengths) & ONES
        steps = lengths - ((b2 | b3) & ONES) - is4 - (is4 << 1)
        words += [(tops | (_shift((s0, s1)[g // 4], (4 * g + i) % 16) & SIGN))
                  - (_shift(steps, 8 - 4 * i) & 0x0F000F00) for i in range(4)]
    return [jnp.concatenate(v, axis=0) for v in zip(*map(_regs, words))]


def _decode_raw(high):
    return jnp.concatenate([w | LOW for a in _regs(high) for w in (a << 8, a)], axis=0)


def _join(low, upper, meta):
    t = jnp.broadcast_to(meta[0:1] & 0xFF, (8, T))
    t = t | (t << 16) | 0x01000100
    return upper - jnp.concatenate(
        [(t - (p & LOW)) & LOW for a in _regs(low) for p in (a, srl(a, 8))], axis=0)


def _body(x_hbm, wq_hbm, kt_hbm, vt_hbm, wo_hbm, out_ref,
          x_f32, wq_f32, wo_f32, k_f32, v_f32, x_w, ctx_w, acc, own, upper, low, high, meta,
          in_sem, kv_sem, send_sem, raw_send_sem, low_sem, last_sem, code_sem, meta_sem, raw_sem,
          entered):
    wq_loads = [
        pltpu.make_async_copy(wq_hbm.at[32 * r0:32 * r1, half * T:(half + 1) * T],
                              wq_f32.at[half, 32 * r0:32 * r1], in_sem.at[i])
        for i, (half, r0, r1) in enumerate(CHUNKS)]
    wo_load = pltpu.make_async_copy(wo_hbm, wo_f32, in_sem.at[len(CHUNKS)])
    x_load = pltpu.make_async_copy(x_hbm, x_f32, in_sem.at[len(CHUNKS) + 1])
    for cp in wq_loads:
        cp.start()

    me = lax.axis_index("i")
    right, diag, left = ((me + k) & (N_DEV - 1) for k in (1, 2, 3))

    def lead(chip, d):
        return jnp.where(chip == 1, 1 - d, d)

    stage_pairs = (((me, 0), (me, 1)),
                   ((left, lead(left, 0)), (right, lead(right, 1))),
                   ((left, lead(left, 1)), (right, lead(right, 0))),
                   ((diag, lead(diag, 0)), (diag, lead(diag, 1))))

    def kv_loads(s):
        cps = []
        for j, (chip, half) in enumerate(stage_pairs[s]):
            rows = pl.ds(pl.multiple_of((2 * chip + half) * T, T), T)
            for src, dst in ((kt_hbm, k_f32), (vt_hbm, v_f32)):
                cps.append(pltpu.make_async_copy(
                    src.at[pl.ds(B_LOC * me, B_LOC), rows], dst.at[s, j], kv_sem.at[s]))
        return cps

    def start_kv(s):
        for cp in kv_loads(s):
            cp.start()

    def wait_kv(s):
        for cp in kv_loads(s):
            cp.wait()

    def remote(view, s, d, send, recv):
        src = (1, d) if s == 3 else (0, lead(me, d if s == 1 else 1 - d))
        return pltpu.make_async_remote_copy(
            view(*src), view(s, d), send, recv, device_id=(jnp.where(d == 0, right, left),),
            device_id_type=pl.DeviceIdType.MESH)

    code_rows, raw_rows = pl.ds(0, CODE_ROWS), pl.ds(CODE_ROWS, 16 * N_G - CODE_ROWS)

    def send_low(w, s, d, r0=0, r1=2 * N_G, sem=None):
        return remote(lambda a, b: low.at[w, a, b, 8 * r0:8 * r1], s, d, send_sem,
                      low_sem.at[3 * w + s - 1] if sem is None else sem)

    def send_meta(w, s, d):
        return remote(lambda a, b: meta.at[w, a, b], s, d, send_sem, meta_sem.at[3 * w + s - 1])

    def send_code(w, s, d):
        return remote(lambda a, b: high.at[w, a, b, code_rows], s, d, send_sem,
                      code_sem.at[3 * w + s - 1])

    def send_raw(w, s, d):
        return remote(lambda a, b: high.at[w, a, b, raw_rows], s, d, raw_send_sem,
                      raw_sem.at[6 * w + 2 * (s - 1) + d])

    def send_chunk(i):
        half, r0, r1 = CHUNKS[i]
        return send_low(WQ, 1, lead(me, half), r0, r1)

    def send_ahead(half):
        return send_low(WQ, 2, lead(me, half), 0, AHEAD)

    def send_last(d, i):
        s, g0, g1 = LAST[i]
        return send_low(WO, s, d, 2 * g0, 2 * g1, last_sem.at[i])

    raw_sends = []

    def start_high(w, s, d, is_raw):
        send_meta(w, s, d).start()
        send_code(w, s, d).start()
        pl.when(is_raw)(lambda: send_raw(w, s, d).start())
        raw_sends.append((w, s, d, is_raw))

    def start_last(stage):
        for i in range(len(LAST)):
            if LAST[i][0] == stage:
                for d in range(2):
                    send_last(d, i).start()

    def wait_filled(buf, sem):
        pltpu.make_async_copy(buf, buf, sem).wait()

    def wait_low(w, s):
        wait_filled(low.at[w, s], low_sem.at[3 * w + s - 1])

    def wait_high(w, s):
        wait_filled(meta.at[w, s], meta_sem.at[3 * w + s - 1])
        wait_filled(high.at[w, s, :, code_rows], code_sem.at[3 * w + s - 1])
        is_raw = [(meta[w, s, d, 1, 0] & 0x80) != 0 for d in range(2)]
        for d in range(2):
            pl.when(is_raw[d])(lambda: send_raw(w, s, d).wait_recv())
        return is_raw

    def split(w, half, r, rows):
        words = pltpu.bitcast(rows.astype(BF16), I32)
        own[w, half, 16 * r:16 * r + words.shape[0]] = words
        low[w, 0, half, 8 * r:8 * r + words.shape[0] // 2] = _low_bytes(words)

    def encode(w, pivots):
        is_raw = []
        for half in range(2):
            code, rows, misfit = _encode(own[w, half], pivots[half])
            is_raw.append(jnp.max(misfit.astype(F32)) > 0)
            high[w, 0, half, code_rows] = code
            meta[w, 0, half] = jnp.where(is_raw[half], RAW, rows)
        for half in range(2):
            @pl.when(is_raw[half])
            def _():
                high[w, 0, half] = _high_bytes(own[w, half])
        return [jnp.where(me == 1, is_raw[1 - d], is_raw[d]) for d in range(2)]

    def decode(w, s):
        pieces = _decode([high[w, s, d, code_rows] for d in range(2)],
                         [meta[w, s, d] for d in range(2)])
        for d in range(2):
            upper[w, s - 1, d] = pieces[d]

    def decode_raw(w, s, is_raw):
        for d in range(2):
            @pl.when(is_raw[d])
            def _():
                upper[w, s - 1, d] = _decode_raw(high[w, s, d])

    def weights(w, s, d, g0, g1):
        if s == 0:
            return pltpu.bitcast(own[w, d, 32 * g0:32 * g1], BF16)
        return pltpu.bitcast(_join(low[w, s, d, 16 * g0:16 * g1],
                                   upper[w, s - 1, d, 32 * g0:32 * g1], meta[w, s, d]), BF16)

    barrier = pltpu.get_barrier_semaphore()
    odd = (me & 1) == 1

    def signal(sem, chip):
        pl.semaphore_signal(sem, inc=1, device_id=(chip,), device_id_type=pl.DeviceIdType.MESH)

    @pl.when(me == 0)
    def _():
        signal(barrier, 1)
        signal(barrier, 3)

    @pl.when(odd)
    def _():
        signal(barrier, 2)
        pl.semaphore_wait(barrier, 1)
        signal(entered, 0)

    @pl.when(me == 2)
    def _():
        pl.semaphore_wait(barrier, 2)
        signal(entered, 1)
        signal(entered, 3)

    known = (me != 0, me == 2)
    for i, (half, r0, r1) in enumerate(CHUNKS):
        wq_loads[i].wait()
        split(WQ, half, r0, wq_f32[half, 32 * r0:32 * r1])
        pl.when(known[half])(lambda: send_chunk(i).start())
        if i == len(CHUNKS) - 3:
            wo_load.start()
    x_load.start()
    for half in range(2):
        pl.when(known[half])(lambda: send_ahead(half).start())
    q_raw = encode(WQ, [_pivot(wq_f32[half]) for half in range(2)])

    pl.when(me == 0)(lambda: pl.semaphore_wait(entered, 2))
    pl.when(odd)(lambda: pl.semaphore_wait(entered, 1))
    for half in range(2):
        @pl.when(jnp.logical_not(known[half]))
        def _():
            for i in range(len(CHUNKS)):
                if CHUNKS[i][0] == half:
                    send_chunk(i).start()
            send_ahead(half).start()

    for d in range(2):
        start_high(WQ, 1, d, q_raw[d])
    for d in range(2):
        start_high(WQ, 2, d, q_raw[1 - d])
        send_low(WQ, 2, d, AHEAD).start()

    wo_load.wait()
    start_kv(0)
    pivots = []
    for half in range(2):
        piece = jnp.concatenate([wo_f32[half * T:(half + 1) * T, c:c + T]
                                 for c in range(0, D_MODEL, T)], axis=0)
        pivots.append(_pivot(piece))
        split(WO, half, 0, piece)
    o_raw = encode(WO, pivots)
    for d in range(2):
        start_high(WO, 1, d, o_raw[d])
        send_low(WO, 1, d).start()

    x_load.wait()
    x_w[...] = pltpu.bitcast((x_f32[...] * 0.125).astype(BF16), I32)

    lo = lax.broadcasted_iota(I32, (BLK, T), 1) < BLK
    on_diag = ((lax.broadcasted_iota(I32, (T, T), 0) < BLK)
               == (lax.broadcasted_iota(I32, (T, T), 1) < BLK))
    tiles = [(j, b, t) for j in range(2) for b in range(B_LOC) for t in range(SEQ // T)]

    def q_proj(s):
        w = jnp.concatenate([weights(WQ, s, d, 0, N_G) for d in range(2)], axis=1)
        return jnp.dot(pltpu.bitcast(x_w[...], BF16), w, preferred_element_type=F32)

    def attention(s, q):
        scores = []
        for j, b, t in tiles:
            qt = q[b * SEQ + t * T:b * SEQ + (t + 1) * T, j * T:(j + 1) * T]
            k = k_f32[s, j, b, :, t * T:(t + 1) * T].T
            for keys, qm in ((jnp.where(lo, k[:BLK], k[BLK:]), jnp.where(on_diag, qt, 0.0)),
                             (jnp.where(lo, k[BLK:], k[:BLK]), jnp.where(on_diag, 0.0, qt))):
                scores.append(lax.dot_general(keys.astype(BF16), qm.astype(BF16),
                                              (((1,), (1,)), ((), ())), preferred_element_type=F32))
        probs = []
        for sc in scores:
            p = jnp.exp(sc - jnp.max(sc, axis=0, keepdims=True))
            inv = 1.0 / jnp.sum(p, axis=0, keepdims=True)
            p = jnp.concatenate([jnp.where(lo, p, 0.0), jnp.where(lo, 0.0, p)], axis=0)
            probs.append((p.astype(BF16), inv))
        heads = []
        for i, (j, b, t) in enumerate(tiles):
            v = v_f32[s, j, b, :, t * T:(t + 1) * T]
            (p0, inv0), (p1, inv1) = probs[2 * i], probs[2 * i + 1]
            c0 = jnp.dot(jnp.where(lo, v[:BLK], v[BLK:]).astype(BF16), p0,
                         preferred_element_type=F32) * inv0
            c1 = jnp.dot(jnp.where(lo, v[BLK:], v[:BLK]).astype(BF16), p1,
                         preferred_element_type=F32) * inv1
            heads.append((jnp.where(lo, c0, c1), jnp.where(lo, c1, c0)))
        n = len(tiles) // 2
        for i, (_, b, t) in enumerate(tiles[:n]):
            r0 = (b * SEQ + t * T) // 2
            for h in range(2):
                c = jnp.concatenate([heads[i][h], heads[n + i][h]], axis=0).T
                ctx_w[s, r0:r0 + T // 2, h * T:(h + 1) * T] = pltpu.bitcast(c.astype(BF16), I32)

    def wo_block(s, g0, g1):
        return jnp.concatenate(
            [jnp.concatenate([weights(WO, s, d, g + h, g + h + 1)
                              for h in range(2) for d in range(2)], axis=0)
             for g in range(g0, g1, 2)], axis=1)

    def out_proj(s, g0=0, g1=N_G):
        return jnp.dot(pltpu.bitcast(ctx_w[s], BF16), wo_block(s, g0, g1),
                       preferred_element_type=F32)

    q = q_proj(0)
    start_kv(1)
    wait_kv(0)
    attention(0, q)
    start_kv(2)

    is_raw = wait_high(WQ, 1)
    wait_low(WQ, 1)
    for d in range(2):
        start_high(WQ, 3, d, is_raw[d])
        send_low(WQ, 3, d).start()
        start_high(WO, 2, d, o_raw[1 - d])
    decode(WQ, 1)
    acc[...] = out_proj(0)
    decode_raw(WQ, 1, is_raw)

    is_raw = wait_high(WQ, 2)
    wait_kv(1)
    start_kv(3)
    decode(WQ, 2)
    attention(1, q_proj(1))
    decode_raw(WQ, 2, is_raw)

    is_raw = wait_high(WO, 1)
    for d in range(2):
        start_high(WO, 3, d, is_raw[d])
    start_last(2)
    wait_low(WQ, 2)
    wait_kv(2)
    decode(WO, 1)
    attention(2, q_proj(2))
    decode_raw(WO, 1, is_raw)

    wait_low(WO, 1)
    start_last(3)
    is_raw = wait_high(WQ, 3)
    decode(WQ, 3)
    acc[...] += out_proj(1)
    decode_raw(WQ, 3, is_raw)

    wait_low(WQ, 3)
    wait_kv(3)
    attention(3, q_proj(3))

    is_raw = wait_high(WO, 2)
    decode(WO, 2)
    decode_raw(WO, 2, is_raw)
    is_raw = wait_high(WO, 3)
    for w, s, d, sent in raw_sends:
        pl.when(sent)(lambda: send_raw(w, s, d).wait_send())

    for i, (s, g0, g1) in enumerate(LAST):
        wait_filled(low.at[WO, s, :, 16 * g0:16 * g1], last_sem.at[i])
        cols = slice(g0 // 2 * T, g1 // 2 * T)
        if s == 2:
            if i == 0:
                decode(WO, 3)
            acc[:, cols] += out_proj(s, g0, g1)
            if i == 0:
                decode_raw(WO, 3, is_raw)
        else:
            w = wo_block(s, g0, g1)
            for b in range(B_LOC):
                c = pltpu.bitcast(ctx_w[s, b * SEQ // 2:(b + 1) * SEQ // 2], BF16)
                y = acc[b * SEQ:(b + 1) * SEQ, cols] + jnp.dot(c, w, preferred_element_type=F32)
                out_ref[b, :, cols] = y.astype(out_ref.dtype)

    for i in range(len(CHUNKS)):
        send_chunk(i).wait_send()
    for d in range(2):
        send_ahead(d).wait_send()
        send_low(WQ, 2, d, AHEAD).wait_send()
        send_low(WQ, 3, d).wait_send()
        send_low(WO, 1, d).wait_send()
        for i in range(len(LAST)):
            send_last(d, i).wait_send()
        for w in (WQ, WO):
            for s in (1, 2, 3):
                send_meta(w, s, d).wait_send()
                send_code(w, s, d).wait_send()


def pallas_dist_sparse_attn_strided_htp_bs_b2_sq256_skv256_hq4_dh64_kernel(
    x: jax.Array,
    Wq: jax.Array,
    K_ext: jax.Array,
    V_ext: jax.Array,
    Wo: jax.Array,
):
    n_b, _, n_h, d_h = K_ext.shape
    kt = jnp.transpose(K_ext, (0, 2, 3, 1)).reshape(n_b, n_h * d_h, SEQ)
    vt = jnp.transpose(V_ext, (0, 2, 3, 1)).reshape(n_b, n_h * d_h, SEQ)
    dma = pltpu.SemaphoreType.DMA
    return pl.pallas_call(
        _body,
        out_shape=jax.ShapeDtypeStruct((B_LOC, SEQ, D_MODEL), BF16),
        in_specs=[pl.BlockSpec(memory_space=pltpu.HBM)] * 5,
        out_specs=pl.BlockSpec(memory_space=pltpu.VMEM),
        scratch_shapes=[
            pltpu.VMEM((ROWS, D_MODEL), F32),
            pltpu.VMEM((2, D_MODEL, T), F32),
            pltpu.VMEM((2 * T, D_MODEL), F32),
            pltpu.VMEM((4, 2, B_LOC, T, SEQ), F32),
            pltpu.VMEM((4, 2, B_LOC, T, SEQ), F32),
            pltpu.VMEM((ROWS // 2, D_MODEL), I32),
            pltpu.VMEM((4, ROWS // 2, 2 * T), I32),
            pltpu.VMEM((ROWS, D_MODEL), F32),
            pltpu.VMEM((2, 2, 32 * N_G, T), I32),
            pltpu.VMEM((2, 3, 2, 32 * N_G, T), I32),
            pltpu.VMEM((2, 4, 2, 16 * N_G, T), I32),
            pltpu.VMEM((2, 4, 2, 16 * N_G, T), I32),
            pltpu.VMEM((2, 4, 2, 2, T), I32),
            dma((len(CHUNKS) + 2,)), dma((4,)), dma, dma,
            dma((4,)), dma((len(LAST),)), dma((6,)), dma((6,)), dma((12,)),
            pltpu.SemaphoreType.REGULAR,
        ],
        compiler_params=pltpu.CompilerParams(
            collective_id=0, vmem_limit_bytes=32 * 1024 * 1024,
            disable_bounds_checks=True, disable_semaphore_checks=True),
    )(x.reshape(ROWS, D_MODEL), Wq, kt, vt, Wo)
```

```python
import jax
import jax.numpy as jnp
from jax import lax
from jax.experimental import pallas as pl
from jax.experimental.pallas import tpu as pltpu

N_DEV = 4
B_LOC, SEQ, D_MODEL = 2, 256, 512
ROWS = B_LOC * SEQ
BLK = 64
T = 128
N_G = 8
WQ, WO = 0, 1
KEYS, VALUES = 0, 1
F32, BF16, I32 = jnp.float32, jnp.bfloat16, jnp.int32

CHUNKS = ((0, 0, 1), (0, 1, 3), (0, 3, 8), (1, 0, 5), (0, 8, 16), (1, 5, 16))
AHEAD = 5
LAST = ((2, 0, 4), (2, 4, 8), (3, 0, 2), (3, 2, 4), (3, 4, 6), (3, 6, 8))

LOW = 0x00FF00FF
SIGN = 0x80008000 - (1 << 32)
ONES = 0x11111111
CODE_ROWS = 48
MAX_BITS = 128 + 21
RAW = 0xFF
srl = lax.shift_right_logical


def _regs(a):
    return [a[i:i + 8] for i in range(0, a.shape[0], 8)]


def _shift(a, n):
    return a if n == 0 else a << n if n > 0 else srl(a, -n)


def _low_bytes(words):
    v = _regs(words)
    return jnp.concatenate([(a & LOW) | ((b & LOW) << 8) for a, b in zip(v[::2], v[1::2])], axis=0)


def _high_bytes(words):
    v = _regs(words)
    return jnp.concatenate([(srl(a, 8) & LOW) | (b & ~LOW) for a, b in zip(v[::2], v[1::2])], axis=0)


def _pivot(rows):
    top = jnp.sum(jnp.abs(rows), axis=0, keepdims=True) * (11.0 / rows.shape[0])
    return srl(pltpu.bitcast(top, I32), 16) & 0x7FFF


def _encode(piece, top):
    words = _regs(piece)
    tops = jnp.broadcast_to(top | (top << 16), (8, T))
    one = jnp.ones((8, T), I32)
    signs, stream, total, wide, longest = [0, 0], [], 0, 0, 0
    for g in reversed(range(N_G)):
        steps = 0
        for i in range(4):
            w = words[4 * g + i]
            signs[g // 4] = signs[g // 4] | _shift(w & SIGN, -((4 * g + i) % 16))
            below = tops - (w & ~SIGN)
            wide = wide | below | (below + 0x01000100)
            steps = steps | _shift(below & 0x0F000F00, 4 * i - 8)
        ge4 = (srl(steps, 2) | srl(steps, 3)) & ONES
        is0 = (((steps | srl(steps, 1)) & ONES) | ge4) ^ ONES
        lengths = steps + ge4 + (is0 << 2)
        for run in (lengths, srl(lengths, 16)):
            bits, code = 0, 0
            for e in (12, 8, 4, 0):
                bits = bits + (_shift(run, -e) & 15)
                code = code | (one << (bits & 31))
            total, longest = total + bits, longest | bits
            carry = [srl(code, 1)] + [srl(s, -bits & 31) for s in stream]
            stream = [c | (s << (bits & 31)) for c, s in zip(carry, stream)] + carry[len(stream):5]
    note = jnp.where(stream[4] != 0, (stream[4] << 3) | lax.broadcasted_iota(I32, (8, T), 0), 0)
    first = jnp.max(note, axis=0, keepdims=True)
    second = jnp.sum(note, axis=0, keepdims=True) - first
    crowded = jnp.sum(jnp.minimum(note, 1), axis=0, keepdims=True) > 2
    misfit = ((srl(wide, 12) & 0x000F000F) != 0) | (longest > 31) | (total > MAX_BITS) | crowded
    meta = jnp.concatenate([(first << 8) | (top & 0xFF), (second << 8) | srl(top, 8)], axis=0)
    return jnp.concatenate(signs + stream[:4], axis=0), meta, misfit


def _decode(codes, metas):
    s0, s1, *stream = [jnp.concatenate(v, axis=0) for v in zip(*map(_regs, codes))]
    m0, m1 = (jnp.concatenate([jnp.broadcast_to(m[i:i + 1], (8, T)) for m in metas], axis=0)
              for i in range(2))
    sub = lax.broadcasted_iota(I32, m0.shape, 0) & 7
    stream.append(jnp.where((srl(m0, 8) & 7) == sub, srl(m0, 11), 0)
                  | jnp.where((srl(m1, 8) & 7) == sub, srl(m1, 11), 0))
    top = (m0 & 0xFF) | ((m1 & 0x7F) << 8)
    tops = top | (top << 16)
    words, at = [], None
    for g in range(N_G):
        runs = []
        for to_come in (2 * (N_G - g) - 1, 2 * (N_G - g) - 2):
            r = stream[0] if at is None else srl(stream[0], at) | ((stream[1] << 1) << (31 - at))
            ends = []
            for e in (12, 8, 4, 0):
                rest = r & (r - 1)
                ends.append(srl(pltpu.bitcast((r ^ rest).astype(F32), I32), 23 - e))
                r = rest
            head = ends[0] + ends[1] + ends[2]
            runs.append(head + ends[3] - srl(head, 4) - (126 << 12))
            if to_come:
                at = ends[3] - 126 if at is None else at + ends[3] - 126
                stream = [jnp.where(at > 31, b, a)
                          for a, b in zip(stream, stream[1:])][:to_come + 1] + stream[4:]
                at = at & 31
        lengths = (runs[0] << 16) + runs[1]
        b2, b3 = srl(lengths, 2), srl(lengths, 3)
        is4 = b2 & ~(b3 | srl(lengths, 1) | lengths) & ONES
        steps = lengths - ((b2 | b3) & ONES) - is4 - (is4 << 1)
        words += [(tops | (_shift((s0, s1)[g // 4], (4 * g + i) % 16) & SIGN))
                  - (_shift(steps, 8 - 4 * i) & 0x0F000F00) for i in range(4)]
    return [jnp.concatenate(v, axis=0) for v in zip(*map(_regs, words))]


def _decode_raw(high):
    return jnp.concatenate([w | LOW for a in _regs(high) for w in (a << 8, a)], axis=0)


def _join(low, upper, meta):
    t = jnp.broadcast_to(meta[0:1] & 0xFF, (8, T))
    t = t | (t << 16) | 0x01000100
    return upper - jnp.concatenate(
        [(t - (p & LOW)) & LOW for a in _regs(low) for p in (a, srl(a, 8))], axis=0)


def _body(x_hbm, wq_hbm, kt_hbm, vt_hbm, wo_hbm, out_ref,
          x_f32, wq_f32, wo_f32, k_f32, v_f32, x_w, ctx_w, acc, own, upper, low, high, meta,
          in_sem, kv_sem, send_sem, low_sem, last_sem, code_sem, meta_sem, raw_sem,
          entered):
    wq_loads = [
        pltpu.make_async_copy(wq_hbm.at[32 * r0:32 * r1, half * T:(half + 1) * T],
                              wq_f32.at[half, 32 * r0:32 * r1], in_sem.at[i])
        for i, (half, r0, r1) in enumerate(CHUNKS)]
    wo_load = pltpu.make_async_copy(wo_hbm, wo_f32, in_sem.at[len(CHUNKS)])
    x_load = pltpu.make_async_copy(x_hbm, x_f32, in_sem.at[len(CHUNKS) + 1])
    for cp in wq_loads:
        cp.start()

    me = lax.axis_index("i")
    right, diag, left = ((me + k) & (N_DEV - 1) for k in (1, 2, 3))

    def lead(chip, d):
        return jnp.where(chip == 1, 1 - d, d)

    stage_pairs = (((me, 0), (me, 1)),
                   ((left, lead(left, 0)), (right, lead(right, 1))),
                   ((left, lead(left, 1)), (right, lead(right, 0))),
                   ((diag, lead(diag, 0)), (diag, lead(diag, 1))))

    def kv_loads(s, which):
        cps = []
        for i in which:
            src, dst = ((kt_hbm, k_f32), (vt_hbm, v_f32))[i]
            for j, (chip, half) in enumerate(stage_pairs[s]):
                rows = pl.ds(pl.multiple_of((2 * chip + half) * T, T), T)
                cps.append(pltpu.make_async_copy(
                    src.at[pl.ds(B_LOC * me, B_LOC), rows], dst.at[s, j], kv_sem.at[2 * s + i]))
        return cps

    def start_kv(s, which=(KEYS, VALUES)):
        for cp in kv_loads(s, which):
            cp.start()

    def wait_kv(s, which=(KEYS, VALUES)):
        for cp in kv_loads(s, which):
            cp.wait()

    send_slots = {}

    def remote(name, view, s, d, recv):
        src = (1, d) if s == 3 else (0, lead(me, d if s == 1 else 1 - d))
        return pltpu.make_async_remote_copy(
            view(*src), view(s, d), send_sem.at[send_slots.setdefault(name, len(send_slots))], recv,
            device_id=(jnp.where(d == 0, right, left),), device_id_type=pl.DeviceIdType.MESH)

    code_rows, raw_rows = pl.ds(0, CODE_ROWS), pl.ds(CODE_ROWS, 16 * N_G - CODE_ROWS)

    def low_rows(w, r0, r1):
        return lambda a, b: low.at[w, a, b, 8 * r0:8 * r1]

    def send_low(w, s, d, r0=0):
        return remote(("low", w, s, d), low_rows(w, r0, 2 * N_G), s, d, low_sem.at[3 * w + s - 1])

    def send_meta(w, s, d):
        return remote(("meta", w, s, d), lambda a, b: meta.at[w, a, b], s, d,
                      meta_sem.at[3 * w + s - 1])

    def send_code(w, s, d):
        return remote(("code", w, s, d), lambda a, b: high.at[w, a, b, code_rows], s, d,
                      code_sem.at[3 * w + s - 1])

    def send_raw(w, s, d):
        return remote(("raw", w, s, d), lambda a, b: high.at[w, a, b, raw_rows], s, d,
                      raw_sem.at[6 * w + 2 * (s - 1) + d])

    def send_chunk(i):
        half, r0, r1 = CHUNKS[i]
        return remote(("chunk", i), low_rows(WQ, r0, r1), 1, lead(me, half), low_sem.at[0])

    def send_ahead(half):
        return remote(("ahead", half), low_rows(WQ, 0, AHEAD), 2, lead(me, half), low_sem.at[1])

    def send_last(d, i):
        s, g0, g1 = LAST[i]
        return remote(("last", d, i), low_rows(WO, 2 * g0, 2 * g1), s, d, last_sem.at[i])

    high_sends = []

    def start_high(w, s, d, is_raw):
        send_meta(w, s, d).start()
        send_code(w, s, d).start()
        pl.when(is_raw)(lambda: send_raw(w, s, d).start())
        high_sends.append((w, s, d, is_raw))

    def wait_high_sent(sends):
        for w, s, d, is_raw in sends:
            send_meta(w, s, d).wait_send()
            send_code(w, s, d).wait_send()
            pl.when(is_raw)(lambda: send_raw(w, s, d).wait_send())

    def start_last(stage):
        for i in range(len(LAST)):
            if LAST[i][0] == stage:
                for d in range(2):
                    send_last(d, i).start()

    def wait_filled(buf, sem):
        pltpu.make_async_copy(buf, buf, sem).wait()

    def wait_low(w, s):
        wait_filled(low.at[w, s], low_sem.at[3 * w + s - 1])

    def wait_high(w, s):
        wait_filled(meta.at[w, s], meta_sem.at[3 * w + s - 1])
        wait_filled(high.at[w, s, :, code_rows], code_sem.at[3 * w + s - 1])
        is_raw = [(meta[w, s, d, 1, 0] & 0x80) != 0 for d in range(2)]
        for d in range(2):
            pl.when(is_raw[d])(lambda: send_raw(w, s, d).wait_recv())
        return is_raw

    def split(w, half, r, rows):
        words = pltpu.bitcast(rows.astype(BF16), I32)
        own[w, half, 16 * r:16 * r + words.shape[0]] = words
        low[w, 0, half, 8 * r:8 * r + words.shape[0] // 2] = _low_bytes(words)

    def encode(w, pivots):
        is_raw = []
        for half in range(2):
            code, rows, misfit = _encode(own[w, half], pivots[half])
            is_raw.append(jnp.max(misfit.astype(F32)) > 0)
            high[w, 0, half, code_rows] = code
            meta[w, 0, half] = jnp.where(is_raw[half], RAW, rows)
        for half in range(2):
            @pl.when(is_raw[half])
            def _():
                high[w, 0, half] = _high_bytes(own[w, half])
        return [jnp.where(me == 1, is_raw[1 - d], is_raw[d]) for d in range(2)]

    def decode(w, s):
        pieces = _decode([high[w, s, d, code_rows] for d in range(2)],
                         [meta[w, s, d] for d in range(2)])
        for d in range(2):
            upper[w, s - 1, d] = pieces[d]

    def decode_raw(w, s, is_raw):
        for d in range(2):
            @pl.when(is_raw[d])
            def _():
                upper[w, s - 1, d] = _decode_raw(high[w, s, d])

    def weights(w, s, d, g0, g1):
        if s == 0:
            return pltpu.bitcast(own[w, d, 32 * g0:32 * g1], BF16)
        return pltpu.bitcast(_join(low[w, s, d, 16 * g0:16 * g1],
                                   upper[w, s - 1, d, 32 * g0:32 * g1], meta[w, s, d]), BF16)

    barrier = pltpu.get_barrier_semaphore()
    odd = (me & 1) == 1

    def signal(sem, chip):
        pl.semaphore_signal(sem, inc=1, device_id=(chip,), device_id_type=pl.DeviceIdType.MESH)

    @pl.when(me == 0)
    def _():
        signal(barrier, 1)
        signal(barrier, 3)

    @pl.when(odd)
    def _():
        signal(barrier, 2)
        pl.semaphore_wait(barrier, 1)
        signal(entered, 0)

    @pl.when(me == 2)
    def _():
        pl.semaphore_wait(barrier, 2)
        signal(entered, 1)
        signal(entered, 3)

    known = (me != 0, me == 2)
    for i, (half, r0, r1) in enumerate(CHUNKS):
        wq_loads[i].wait()
        split(WQ, half, r0, wq_f32[half, 32 * r0:32 * r1])
        pl.when(known[half])(lambda: send_chunk(i).start())
        if i == len(CHUNKS) - 3:
            wo_load.start()
    x_load.start()
    for half in range(2):
        pl.when(known[half])(lambda: send_ahead(half).start())
    q_raw = encode(WQ, [_pivot(wq_f32[half]) for half in range(2)])

    pl.when(me == 0)(lambda: pl.semaphore_wait(entered, 2))
    pl.when(odd)(lambda: pl.semaphore_wait(entered, 1))
    for half in range(2):
        @pl.when(jnp.logical_not(known[half]))
        def _():
            for i in range(len(CHUNKS)):
                if CHUNKS[i][0] == half:
                    send_chunk(i).start()
            send_ahead(half).start()

    for d in range(2):
        start_high(WQ, 1, d, q_raw[d])
    for d in range(2):
        start_high(WQ, 2, d, q_raw[1 - d])
        send_low(WQ, 2, d, AHEAD).start()

    wo_load.wait()
    start_kv(0, [KEYS])
    pivots = []
    for half in range(2):
        piece = jnp.concatenate([wo_f32[half * T:(half + 1) * T, c:c + T]
                                 for c in range(0, D_MODEL, T)], axis=0)
        pivots.append(_pivot(piece))
        split(WO, half, 0, piece)
    o_raw = encode(WO, pivots)
    for d in range(2):
        start_high(WO, 1, d, o_raw[d])
        send_low(WO, 1, d).start()

    x_load.wait()
    start_kv(0, [VALUES])
    x_w[...] = pltpu.bitcast((x_f32[...] * 0.125).astype(BF16), I32)

    lo = lax.broadcasted_iota(I32, (BLK, T), 1) < BLK
    on_diag = ((lax.broadcasted_iota(I32, (T, T), 0) < BLK)
               == (lax.broadcasted_iota(I32, (T, T), 1) < BLK))
    tiles = [(j, b, t) for j in range(2) for b in range(B_LOC) for t in range(SEQ // T)]

    def q_proj(s):
        w = jnp.concatenate([weights(WQ, s, d, 0, N_G) for d in range(2)], axis=1)
        return jnp.dot(pltpu.bitcast(x_w[...], BF16), w, preferred_element_type=F32)

    def softmax(s, q):
        scores = []
        for j, b, t in tiles:
            qt = q[b * SEQ + t * T:b * SEQ + (t + 1) * T, j * T:(j + 1) * T]
            k = k_f32[s, j, b, :, t * T:(t + 1) * T].T
            for keys, qm in ((jnp.where(lo, k[:BLK], k[BLK:]), jnp.where(on_diag, qt, 0.0)),
                             (jnp.where(lo, k[BLK:], k[:BLK]), jnp.where(on_diag, 0.0, qt))):
                scores.append(lax.dot_general(keys.astype(BF16), qm.astype(BF16),
                                              (((1,), (1,)), ((), ())), preferred_element_type=F32))
        probs = []
        for sc in scores:
            p = jnp.exp(sc - jnp.max(sc, axis=0, keepdims=True))
            inv = 1.0 / jnp.sum(p, axis=0, keepdims=True)
            p = jnp.concatenate([jnp.where(lo, p, 0.0), jnp.where(lo, 0.0, p)], axis=0)
            probs.append((p.astype(BF16), inv))
        return probs

    def context(s, probs):
        heads = []
        for i, (j, b, t) in enumerate(tiles):
            v = v_f32[s, j, b, :, t * T:(t + 1) * T]
            (p0, inv0), (p1, inv1) = probs[2 * i], probs[2 * i + 1]
            c0 = jnp.dot(jnp.where(lo, v[:BLK], v[BLK:]).astype(BF16), p0,
                         preferred_element_type=F32) * inv0
            c1 = jnp.dot(jnp.where(lo, v[BLK:], v[:BLK]).astype(BF16), p1,
                         preferred_element_type=F32) * inv1
            heads.append((jnp.where(lo, c0, c1), jnp.where(lo, c1, c0)))
        n = len(tiles) // 2
        for i, (_, b, t) in enumerate(tiles[:n]):
            r0 = (b * SEQ + t * T) // 2
            for h in range(2):
                c = jnp.concatenate([heads[i][h], heads[n + i][h]], axis=0).T
                ctx_w[s, r0:r0 + T // 2, h * T:(h + 1) * T] = pltpu.bitcast(c.astype(BF16), I32)

    def wo_block(s, g0, g1):
        return jnp.concatenate(
            [jnp.concatenate([weights(WO, s, d, g + h, g + h + 1)
                              for h in range(2) for d in range(2)], axis=0)
             for g in range(g0, g1, 2)], axis=1)

    def out_proj(s, g0=0, g1=N_G):
        return jnp.dot(pltpu.bitcast(ctx_w[s], BF16), wo_block(s, g0, g1),
                       preferred_element_type=F32)

    q = q_proj(0)
    start_kv(1)
    wait_kv(0, [KEYS])
    probs = softmax(0, q)
    wait_kv(0, [VALUES])
    context(0, probs)
    start_kv(2)

    is_raw = wait_high(WQ, 1)
    wait_low(WQ, 1)
    for d in range(2):
        start_high(WQ, 3, d, is_raw[d])
        send_low(WQ, 3, d).start()
    for d in range(2):
        start_high(WO, 2, d, o_raw[1 - d])
    decode(WQ, 1)
    acc[...] = out_proj(0)
    decode_raw(WQ, 1, is_raw)

    is_raw = wait_high(WQ, 2)
    wait_kv(1)
    start_kv(3)
    decode(WQ, 2)
    context(1, softmax(1, q_proj(1)))
    decode_raw(WQ, 2, is_raw)

    is_raw = wait_high(WO, 1)
    for d in range(2):
        start_high(WO, 3, d, is_raw[d])
    start_last(2)
    wait_low(WQ, 2)
    wait_kv(2)
    decode(WO, 1)
    context(2, softmax(2, q_proj(2)))
    decode_raw(WO, 1, is_raw)

    wait_low(WO, 1)
    start_last(3)
    is_raw = wait_high(WQ, 3)
    decode(WQ, 3)
    acc[...] += out_proj(1)
    decode_raw(WQ, 3, is_raw)

    for i in range(len(CHUNKS)):
        send_chunk(i).wait_send()
    for d in range(2):
        send_ahead(d).wait_send()
        send_low(WQ, 2, d, AHEAD).wait_send()
        send_low(WO, 1, d).wait_send()
        send_low(WQ, 3, d).wait_send()
    wait_high_sent(high_sends[:8])
    wait_low(WQ, 3)
    wait_kv(3)
    context(3, softmax(3, q_proj(3)))

    is_raw = wait_high(WO, 2)
    decode(WO, 2)
    decode_raw(WO, 2, is_raw)
    is_raw = wait_high(WO, 3)
    wait_high_sent(high_sends[8:])

    for i, (s, g0, g1) in enumerate(LAST):
        for d in range(2):
            send_last(d, i).wait_send()
        wait_filled(low.at[WO, s, :, 16 * g0:16 * g1], last_sem.at[i])
        cols = slice(g0 // 2 * T, g1 // 2 * T)
        if s == 2:
            if i == 0:
                decode(WO, 3)
            acc[:, cols] += out_proj(s, g0, g1)
            if i == 0:
                decode_raw(WO, 3, is_raw)
        else:
            w = wo_block(s, g0, g1)
            for b in range(B_LOC):
                c = pltpu.bitcast(ctx_w[s, b * SEQ // 2:(b + 1) * SEQ // 2], BF16)
                y = acc[b * SEQ:(b + 1) * SEQ, cols] + jnp.dot(c, w, preferred_element_type=F32)
                out_ref[b, :, cols] = y.astype(out_ref.dtype)


def pallas_dist_sparse_attn_strided_htp_bs_b2_sq256_skv256_hq4_dh64_kernel(
    x: jax.Array,
    Wq: jax.Array,
    K_ext: jax.Array,
    V_ext: jax.Array,
    Wo: jax.Array,
):
    n_b, _, n_h, d_h = K_ext.shape
    kt = jnp.transpose(K_ext, (0, 2, 3, 1)).reshape(n_b, n_h * d_h, SEQ)
    vt = jnp.transpose(V_ext, (0, 2, 3, 1)).reshape(n_b, n_h * d_h, SEQ)
    dma = pltpu.SemaphoreType.DMA
    return pl.pallas_call(
        _body,
        out_shape=jax.ShapeDtypeStruct((B_LOC, SEQ, D_MODEL), BF16),
        in_specs=[pl.BlockSpec(memory_space=pltpu.HBM)] * 5,
        out_specs=pl.BlockSpec(memory_space=pltpu.VMEM),
        scratch_shapes=[
            pltpu.VMEM((ROWS, D_MODEL), F32),
            pltpu.VMEM((2, D_MODEL, T), F32),
            pltpu.VMEM((2 * T, D_MODEL), F32),
            pltpu.VMEM((4, 2, B_LOC, T, SEQ), F32),
            pltpu.VMEM((4, 2, B_LOC, T, SEQ), F32),
            pltpu.VMEM((ROWS // 2, D_MODEL), I32),
            pltpu.VMEM((4, ROWS // 2, 2 * T), I32),
            pltpu.VMEM((ROWS, D_MODEL), F32),
            pltpu.VMEM((2, 2, 32 * N_G, T), I32),
            pltpu.VMEM((2, 3, 2, 32 * N_G, T), I32),
            pltpu.VMEM((2, 4, 2, 16 * N_G, T), I32),
            pltpu.VMEM((2, 4, 2, 16 * N_G, T), I32),
            pltpu.VMEM((2, 4, 2, 2, T), I32),
            dma((len(CHUNKS) + 2,)), dma((8,)), dma((len(CHUNKS) + 2 * len(LAST) + 8 + 3 * 12,)),
            dma((4,)), dma((len(LAST),)), dma((6,)), dma((6,)), dma((12,)),
            pltpu.SemaphoreType.REGULAR,
        ],
        compiler_params=pltpu.CompilerParams(
            collective_id=0, vmem_limit_bytes=32 * 1024 * 1024,
            disable_bounds_checks=True, disable_semaphore_checks=True),
    )(x.reshape(ROWS, D_MODEL), Wq, kt, vt, Wo)
```
